```python
import numpy as np

kernel_name = "dist_ag_xy_y_m1024_n512"

def setup_inputs():
    return {"x": np.random.randn(2048, 512).astype(np.float32)}

def reference(x: np.ndarray) -> np.ndarray:
    return x
```

```python
import jax
import jax.numpy as jnp
from jax import lax
from jax.experimental import pallas as pl
from jax.experimental.pallas import tpu as pltpu

CHUNK = 16
FWD_ROWS = 480
SEND_AHEAD = 10
X_RECV_LAG = 10


def pallas_dist_ag_xy_y_m1024_n512_kernel(
    x: jax.Array,
):
    m, n = x.shape
    fwd_rows = FWD_ROWS
    direct_rows = m - fwd_rows
    n_fwd = fwd_rows // CHUNK
    n_direct = direct_rows // CHUNK
    assert n_fwd * CHUNK == fwd_rows and n_direct * CHUNK == direct_rows
    assert n_fwd <= n_direct
    mesh_id = pl.DeviceIdType.MESH

    def kernel_body(
        x_ref, o_ref, send_buf, y_buf, x_buf,
        load_sems, rest_sem, y_send_sem, y_recv_sems, x_send_sem, x_recv_sems,
    ):
        my_x = lax.axis_index("x")
        my_y = lax.axis_index("y")
        y_nbr = (my_x, 1 - my_y)
        x_nbr = (1 - my_x, my_y)

        barrier_sem = pltpu.get_barrier_semaphore()
        for nbr in (y_nbr, x_nbr):
            pl.semaphore_signal(barrier_sem, inc=1, device_id=nbr, device_id_type=mesh_id)

        def shard_row(c, col):
            if c < n_fwd:
                return col * direct_rows + c * CHUNK
            return c * CHUNK

        def rows(start, size=CHUNK):
            return pl.ds(pl.multiple_of(start, CHUNK), size)

        def buf_rows(c):
            return pl.ds(c * CHUNK, CHUNK)

        own = my_y * m
        other = (1 - my_y) * m

        loads = [
            pltpu.make_async_copy(
                x_ref.at[rows(shard_row(c, my_x))],
                o_ref.at[rows(own + shard_row(c, my_x))],
                load_sems.at[c],
            )
            for c in range(n_direct)
        ]
        rest = pltpu.make_async_copy(
            x_ref.at[rows((1 - my_x) * direct_rows, fwd_rows)],
            o_ref.at[rows(own + (1 - my_x) * direct_rows, fwd_rows)],
            rest_sem,
        )
        for load in loads:
            load.start()
        rest.start()

        y_copies = [
            pltpu.make_async_remote_copy(
                send_buf.at[buf_rows(c)], y_buf.at[buf_rows(c)],
                y_send_sem, y_recv_sems.at[c],
                device_id=y_nbr, device_id_type=mesh_id,
            )
            for c in range(n_direct)
        ]
        x_copies = [
            pltpu.make_async_remote_copy(
                y_buf.at[buf_rows(c)], x_buf.at[buf_rows(c)],
                x_send_sem, x_recv_sems.at[c],
                device_id=x_nbr, device_id_type=mesh_id,
            )
            for c in range(n_fwd)
        ]

        def send(c):
            loads[c].wait()
            send_buf[buf_rows(c), :] = o_ref[
                rows(own + shard_row(c, my_x)), :
            ].astype(send_buf.dtype)
            if c == 0:
                pl.semaphore_wait(barrier_sem, 2)
            y_copies[c].start()

        def recv_y(c):
            y_copies[c].wait_recv()
            if c < n_fwd:
                x_copies[c].start()
            o_ref[rows(other + shard_row(c, my_x)), :] = y_buf[
                buf_rows(c), :
            ].astype(o_ref.dtype)

        def recv_x(c):
            x_copies[c].wait_recv()
            o_ref[rows(other + shard_row(c, 1 - my_x)), :] = x_buf[
                buf_rows(c), :
            ].astype(o_ref.dtype)

        for c in range(min(SEND_AHEAD, n_direct)):
            send(c)
        for c in range(n_direct):
            recv_y(c)
            if c + SEND_AHEAD < n_direct:
                send(c + SEND_AHEAD)
            if 0 <= c - X_RECV_LAG < n_fwd:
                recv_x(c - X_RECV_LAG)
        for c in range(max(n_direct - X_RECV_LAG, 0), n_fwd):
            recv_x(c)

        pltpu.make_async_remote_copy(
            send_buf, send_buf, y_send_sem, y_recv_sems.at[0],
            device_id=y_nbr, device_id_type=mesh_id,
        ).wait_send()
        pltpu.make_async_remote_copy(
            x_buf, x_buf, x_send_sem, x_recv_sems.at[0],
            device_id=x_nbr, device_id_type=mesh_id,
        ).wait_send()
        rest.wait()

    out_shape = jax.ShapeDtypeStruct((2 * m, n), x.dtype)
    return pl.pallas_call(
        kernel_body,
        out_shape=out_shape,
        in_specs=[pl.BlockSpec(memory_space=pltpu.HBM)],
        out_specs=pl.BlockSpec(memory_space=pltpu.VMEM),
        scratch_shapes=[
            pltpu.VMEM((direct_rows, n), jnp.bfloat16),
            pltpu.VMEM((direct_rows, n), jnp.bfloat16),
            pltpu.VMEM((fwd_rows, n), jnp.bfloat16),
            pltpu.SemaphoreType.DMA((n_direct,)),
            pltpu.SemaphoreType.DMA,
            pltpu.SemaphoreType.DMA,
            pltpu.SemaphoreType.DMA((n_direct,)),
            pltpu.SemaphoreType.DMA,
            pltpu.SemaphoreType.DMA((n_fwd,)),
        ],
        compiler_params=pltpu.CompilerParams(
            collective_id=0, disable_semaphore_checks=True
        ),
    )(x)
```

```python
import jax
import jax.numpy as jnp
from jax import lax
from jax.experimental import pallas as pl
from jax.experimental.pallas import tpu as pltpu

CHUNK = 16
FWD_ROWS = 464
SEND_AHEAD = 10
X_RECV_LAG = 10
LOAD_AHEAD = 16


def pallas_dist_ag_xy_y_m1024_n512_kernel(
    x: jax.Array,
):
    m, n = x.shape
    fwd_rows = FWD_ROWS
    direct_rows = m - fwd_rows
    n_fwd = fwd_rows // CHUNK
    n_direct = direct_rows // CHUNK
    assert n_fwd * CHUNK == fwd_rows and n_direct * CHUNK == direct_rows
    assert n_fwd <= n_direct
    mesh_id = pl.DeviceIdType.MESH

    def kernel_body(
        x_ref, o_ref, send_buf, y_buf, x_buf,
        load_sems, rest_sem, y_send_sem, y_recv_sems, x_send_sem, x_recv_sems,
        relay_sem,
    ):
        my_x = lax.axis_index("x")
        my_y = lax.axis_index("y")
        y_nbr = (my_x, 1 - my_y)
        x_nbr = (1 - my_x, my_y)

        def shard_row(c, col):
            if c < n_fwd:
                return col * direct_rows + c * CHUNK
            return c * CHUNK

        def rows(start, size=CHUNK):
            return pl.ds(pl.multiple_of(start, CHUNK), size)

        def buf_rows(c):
            return pl.ds(c * CHUNK, CHUNK)

        own = my_y * m
        other = (1 - my_y) * m

        loads = [
            pltpu.make_async_copy(
                x_ref.at[rows(shard_row(c, my_x))],
                o_ref.at[rows(own + shard_row(c, my_x))],
                load_sems.at[c],
            )
            for c in range(n_direct)
        ]
        rest = pltpu.make_async_copy(
            x_ref.at[rows((1 - my_x) * direct_rows, fwd_rows)],
            o_ref.at[rows(own + (1 - my_x) * direct_rows, fwd_rows)],
            rest_sem,
        )
        loads[0].start()

        def at(col, row):
            return jnp.logical_and(my_x == col, my_y == row)

        def signal(sem, nbr):
            pl.semaphore_signal(sem, inc=1, device_id=nbr, device_id_type=mesh_id)

        barrier_sem = pltpu.get_barrier_semaphore()
        signal(barrier_sem, y_nbr)
        pl.when(jnp.logical_not(at(1, 1)))(lambda: signal(barrier_sem, x_nbr))

        for load in loads[1:LOAD_AHEAD]:
            load.start()

        y_copies = [
            pltpu.make_async_remote_copy(
                send_buf.at[buf_rows(c)], y_buf.at[buf_rows(c)],
                y_send_sem, y_recv_sems.at[c],
                device_id=y_nbr, device_id_type=mesh_id,
            )
            for c in range(n_direct)
        ]
        x_copies = [
            pltpu.make_async_remote_copy(
                y_buf.at[buf_rows(c)], x_buf.at[buf_rows(c)],
                x_send_sem, x_recv_sems.at[c],
                device_id=x_nbr, device_id_type=mesh_id,
            )
            for c in range(n_fwd)
        ]

        def send(c):
            loads[c].wait()
            send_buf[buf_rows(c), :] = o_ref[
                rows(own + shard_row(c, my_x)), :
            ].astype(send_buf.dtype)
            if c == 0:
                pl.when(at(0, 1))(lambda: pl.semaphore_wait(barrier_sem, 1))
                pl.when(jnp.logical_not(at(0, 1)))(
                    lambda: pl.semaphore_wait(barrier_sem, 2)
                )
            y_copies[c].start()
            if c == 0:
                pl.when(at(1, 0))(lambda: signal(relay_sem, x_nbr))
            if c + LOAD_AHEAD < n_direct:
                loads[c + LOAD_AHEAD].start()
            if c == n_direct - 1:
                rest.start()

        def recv_y(c):
            y_copies[c].wait_recv()
            if c < n_fwd:
                x_copies[c].start()
            o_ref[rows(other + shard_row(c, my_x)), :] = y_buf[
                buf_rows(c), :
            ].astype(o_ref.dtype)

        def recv_x(c):
            x_copies[c].wait_recv()
            o_ref[rows(other + shard_row(c, 1 - my_x)), :] = x_buf[
                buf_rows(c), :
            ].astype(o_ref.dtype)

        for c in range(min(SEND_AHEAD, n_direct)):
            send(c)
        pl.when(my_x == 0)(lambda: pl.semaphore_wait(relay_sem, 1))
        pl.when(at(0, 0))(lambda: signal(relay_sem, y_nbr))
        for c in range(n_direct):
            recv_y(c)
            if c + SEND_AHEAD < n_direct:
                send(c + SEND_AHEAD)
            if 0 <= c - X_RECV_LAG < n_fwd:
                recv_x(c - X_RECV_LAG)
        for c in range(max(n_direct - X_RECV_LAG, 0), n_fwd):
            recv_x(c)

        pltpu.make_async_remote_copy(
            send_buf, send_buf, y_send_sem, y_recv_sems.at[0],
            device_id=y_nbr, device_id_type=mesh_id,
        ).wait_send()
        pltpu.make_async_remote_copy(
            x_buf, x_buf, x_send_sem, x_recv_sems.at[0],
            device_id=x_nbr, device_id_type=mesh_id,
        ).wait_send()
        rest.wait()

    out_shape = jax.ShapeDtypeStruct((2 * m, n), x.dtype)
    return pl.pallas_call(
        kernel_body,
        out_shape=out_shape,
        in_specs=[pl.BlockSpec(memory_space=pltpu.HBM)],
        out_specs=pl.BlockSpec(memory_space=pltpu.VMEM),
        scratch_shapes=[
            pltpu.VMEM((direct_rows, n), jnp.bfloat16),
            pltpu.VMEM((direct_rows, n), jnp.bfloat16),
            pltpu.VMEM((fwd_rows, n), jnp.bfloat16),
            pltpu.SemaphoreType.DMA((n_direct,)),
            pltpu.SemaphoreType.DMA,
            pltpu.SemaphoreType.DMA,
            pltpu.SemaphoreType.DMA((n_direct,)),
            pltpu.SemaphoreType.DMA,
            pltpu.SemaphoreType.DMA((n_fwd,)),
            pltpu.SemaphoreType.REGULAR,
        ],
        compiler_params=pltpu.CompilerParams(
            collective_id=0, disable_semaphore_checks=True
        ),
    )(x)
```
